```python
import numpy as np

kernel_name = "dist_sparse_attn_causalblk_htp_bs_b2_sq256_skv256_hq4_dh64"

def setup_inputs():
    x = np.random.randn(8, 256, 512).astype(np.float32)
    Wq = np.random.randn(512, 1024).astype(np.float32) * 0.02
    K_ext = np.random.randn(8, 256, 16, 64).astype(np.float32)
    V_ext = np.random.randn(8, 256, 16, 64).astype(np.float32)
    Wo = np.random.randn(1024, 512).astype(np.float32) * 0.02
    return {"x": x, "Wq": Wq, "K_ext": K_ext, "V_ext": V_ext, "Wo": Wo}

def reference(x, Wq, K_ext, V_ext, Wo):
    B, Sq, Skv, Hq, Dh = 8, 256, 256, 16, 64
    Q = (x @ Wq).reshape(B, Sq, Hq, Dh)
    qb = (np.arange(Sq) // 64)[:, None]
    kb = (np.arange(Skv) // 64)[None, :]
    mask = kb <= qb
    scores = np.einsum('bihd,bjhd->bhij', Q, K_ext).astype(np.float32) * 0.125
    scores = np.where(mask[None, None, :, :], scores, -1e9)
    scores_max = scores.max(axis=-1, keepdims=True)
    w = np.exp(scores - scores_max)
    row_keep = mask.any(axis=1)
    w_sum = np.where(row_keep[None, None, :, None], w.sum(axis=-1, keepdims=True), 1.0)
    w = w / w_sum
    w = np.where(row_keep[None, None, :, None], w, 0.0)
    ctx = np.einsum('bhij,bjhd->bihd', w, V_ext).reshape(B, Sq, Hq * Dh)
    return ctx @ Wo
```

```python
import contextlib
import functools
import math

import jax
import jax.numpy as jnp
from jax import lax
from jax.experimental import pallas as pl
from jax.experimental.pallas import tpu as pltpu

N_DEV = 4
B_LOC, SQ, DM = 2, 256, 512
DH, BLK = 64, 64
NBLK = SQ // BLK
TOK = B_LOC * SQ
Q_SCALE = 0.125 * math.log2(math.e)
BF, F32 = jnp.bfloat16, jnp.float32
MESH = pl.DeviceIdType.MESH

OWN, LEFT, RIGHT, DIAG = 0, 1, 2, 3


def make(scopes=False, comm=True, asym=True, wq_rows=(32, 96, 128, 256), tail=4, mxu_sum=False):
    scope = jax.named_scope if scopes else (lambda name: contextlib.nullcontext())

    def body(x_hbm, wq_hbm, k_hbm, v_hbm, wo_hbm, out_ref,
             x_f, wq_f, wo_f, k_f, v_f,
             xb, wq, wo, kbd, vbd, ctx, acc,
             ld_sem, q_send, q_recv, o_send, o_recv, go_sem):
        me = lax.axis_index("i")
        left, right, diag = (me + 3) % N_DEV, (me + 1) % N_DEV, (me + 2) % N_DEV
        odd = me % 2 == 1

        if comm:
            bar = pltpu.get_barrier_semaphore()

            def sig():
                for n in (left, right):
                    pl.semaphore_signal(bar, inc=1, device_id=(n,), device_id_type=MESH)
            if asym:
                pl.when(me != 2)(sig)
            else:
                sig()

        n_ld = [0]

        def load(src, dst):
            c = pltpu.make_async_copy(src, dst, ld_sem.at[n_ld[0]])
            n_ld[0] += 1
            c.start()
            return c

        offs = [sum(wq_rows[:i]) for i in range(len(wq_rows))]
        wq_ld = [load(wq_hbm.at[pl.ds(o, r)], wq_f.at[pl.ds(o, r)]) for o, r in zip(offs, wq_rows)]
        wo_ld = load(wo_hbm, wo_f)
        x_ld = load(x_hbm, x_f)
        kv_ld = []
        for slot, src in ((OWN, me), (LEFT, left), (RIGHT, right), (DIAG, diag)):
            rows = pl.ds(pl.multiple_of(src * 256, 256), 256)
            kv_ld.append((load(k_hbm.at[pl.ds(me * B_LOC, B_LOC), rows], k_f.at[slot]),
                          load(v_hbm.at[pl.ds(me * B_LOC, B_LOC), rows], v_f.at[slot])))

        tgt = (right, left)
        land = (LEFT, RIGHT)

        def rdma(src, dst, ss, rs, d):
            return pltpu.make_async_remote_copy(src, dst, ss, rs, device_id=(tgt[d],), device_id_type=MESH)

        nq = len(wq_rows)

        def q_first(d, i):
            r = pl.ds(offs[i], wq_rows[i])
            return rdma(wq.at[OWN, d, r], wq.at[land[d], d, r], q_send.at[d, i], q_recv.at[d, i], d)

        def q_second(d):
            return rdma(wq.at[OWN, 1 - d], wq.at[land[d], 1 - d], q_send.at[d, nq], q_recv.at[d, nq], d)

        def q_fwd(d):
            return rdma(wq.at[land[d], d], wq.at[DIAG, d], q_send.at[d, nq + 1], q_recv.at[d, nq + 1], d)

        def o_first(d):
            return rdma(wo.at[OWN, d], wo.at[land[d], d], o_send.at[d, 0], o_recv.at[d, 0], d)

        def o_second(d):
            return rdma(wo.at[OWN, 1 - d], wo.at[land[d], 1 - d], o_send.at[d, 1], o_recv.at[d, 1], d)

        tw = DM // tail

        def o_fwd(d, j):
            c = pl.ds(j * tw, tw)
            return rdma(wo.at[land[d], d, :, c], wo.at[DIAG, d, :, c], o_send.at[d, 2 + j], o_recv.at[d, 2 + j], d)

        if comm:
            with scope("barrier"):
                if asym:
                    pl.semaphore_wait(bar, jnp.where(odd, 1, 2))

                    @pl.when(me == 2)
                    def _():
                        for n in (left, right):
                            pl.semaphore_signal(go_sem, inc=1, device_id=(n,), device_id_type=MESH)
                else:
                    pl.semaphore_wait(bar, 2)

        now = (me != 1, me != 3) if asym else (True, True)
        with scope("wq_send"):
            for i in range(nq):
                wq_ld[i].wait()
                r = pl.ds(offs[i], wq_rows[i])
                w = (wq_f[r, :] * Q_SCALE).astype(BF)
                wq[OWN, 0, r, :] = w[:, :128]
                wq[OWN, 1, r, :] = w[:, 128:]
                if comm:
                    for d in range(2):
                        pl.when(now[d])(q_first(d, i).start)
            if comm and asym:
                @pl.when(odd)
                def _():
                    pl.semaphore_wait(go_sem, 1)
                for d in range(2):
                    @pl.when(jnp.logical_not(now[d]))
                    def _():
                        for i in range(nq):
                            q_first(d, i).start()
            if comm:
                for d in range(2):
                    q_second(d).start()

        with scope("prep"):
            wo_ld.wait()
            for h in range(2):
                wo[OWN, h] = wo_f[pl.ds(h * 128, 128), :].astype(BF)
            x_ld.wait()
            for b in range(B_LOC):
                xb[pl.ds(b * SQ, SQ), :] = x_f[b].astype(BF)

        lane_lo = lax.broadcasted_iota(jnp.int32, (BLK, 128), 1) < DH

        def prep_kv(slot):
            for ld, src, dst in ((kv_ld[slot][0], k_f, kbd), (kv_ld[slot][1], v_f, vbd)):
                ld.wait()
                for b in range(B_LOC):
                    for h in range(2):
                        for j in range(2):
                            ta = src[slot, b, pl.ds(h * 128, DH), pl.ds(j * 128, 128)]
                            tb = src[slot, b, pl.ds(h * 128 + DH, DH), pl.ds(j * 128, 128)]
                            ra, rb = pltpu.roll(ta, DH, 1), pltpu.roll(tb, DH, 1)
                            dst[slot, h, b, 2 * j, pl.ds(0, DH)] = jnp.where(lane_lo, ta, 0.0).astype(BF)
                            dst[slot, h, b, 2 * j, pl.ds(DH, DH)] = jnp.where(lane_lo, 0.0, rb).astype(BF)
                            dst[slot, h, b, 2 * j + 1, pl.ds(0, DH)] = jnp.where(lane_lo, ra, 0.0).astype(BF)
                            dst[slot, h, b, 2 * j + 1, pl.ds(DH, DH)] = jnp.where(lane_lo, 0.0, tb).astype(BF)

        def seg(red, fill, t):
            a = red(jnp.where(lane_lo, t, fill), axis=1, keepdims=True)
            c = red(jnp.where(lane_lo, fill, t), axis=1, keepdims=True)
            return jnp.where(lane_lo, a, c)

        def attend(slot, h):
            q = jnp.dot(xb[...], wq[slot, h], preferred_element_type=F32).astype(BF)
            for b in range(B_LOC):
                s = [jnp.dot(q[b * SQ + kb * BLK:(b + 1) * SQ], kbd[slot, h, b, kb],
                             preferred_element_type=F32) for kb in range(NBLK)]
                p = [[None] * NBLK for _ in range(NBLK)]
                inv = []
                for qb in range(NBLK):
                    t = [s[kb][(qb - kb) * BLK:(qb - kb + 1) * BLK] for kb in range(qb + 1)]
                    m = seg(jnp.max, -jnp.inf, functools.reduce(jnp.maximum, t))
                    e = [jnp.exp2(u - m) for u in t]
                    inv.append(1.0 / seg(jnp.sum, 0.0, functools.reduce(jnp.add, e)))
                    for kb in range(qb + 1):
                        p[kb][qb] = e[kb].astype(BF)
                o = [lax.dot_general(jnp.concatenate(p[kb][kb:], axis=0), vbd[slot, h, b, kb],
                                     (((1,), (1,)), ((), ())), preferred_element_type=F32)
                     for kb in range(NBLK)]
                for qb in range(NBLK):
                    c = functools.reduce(
                        jnp.add, [o[kb][(qb - kb) * BLK:(qb - kb + 1) * BLK] for kb in range(qb + 1)])
                    ctx[slot, h, pl.ds(b * SQ + qb * BLK, BLK), :] = (c * inv[qb]).astype(BF)

        def proj(parts, cols=slice(None)):
            return functools.reduce(jnp.add, [
                jnp.dot(ctx[s, h], wo[s, h, :, cols], preferred_element_type=F32) for s, h in parts])

        with scope("own"):
            prep_kv(OWN)
            attend(OWN, 0)
        with scope("w1"):
            if comm:
                for d in range(2):
                    for i in range(nq):
                        q_first(d, i).wait_recv()
                for d in range(2):
                    q_fwd(d).start()
                for d in range(2):
                    o_first(d).start()
                for d in range(2):
                    o_second(d).start()
        with scope("a1"):
            attend(OWN, 1)
            prep_kv(LEFT)
            prep_kv(RIGHT)
            attend(LEFT, 0)
            attend(RIGHT, 1)
        with scope("w2"):
            if comm:
                for d in range(2):
                    q_second(d).wait_recv()
        with scope("a2"):
            attend(LEFT, 1)
            attend(RIGHT, 0)
            prep_kv(DIAG)
        with scope("w3"):
            if comm:
                for d in range(2):
                    q_fwd(d).wait_recv()
        with scope("a3"):
            attend(DIAG, 0)
        with scope("w4"):
            if comm:
                for d in range(2):
                    o_first(d).wait_recv()
                for j in range(tail):
                    for d in range(2):
                        o_fwd(d, j).start()
        with scope("o1"):
            attend(DIAG, 1)
            acc[...] = proj([(OWN, 0), (OWN, 1), (LEFT, 0), (RIGHT, 1)])
        with scope("w5"):
            if comm:
                for d in range(2):
                    o_second(d).wait_recv()
        with scope("o2"):
            acc[...] += proj([(LEFT, 1), (RIGHT, 0)])
        if comm:
            for d in range(2):
                for i in range(nq):
                    q_first(d, i).wait_send()
                q_second(d).wait_send()
                q_fwd(d).wait_send()
                o_first(d).wait_send()
                o_second(d).wait_send()
        for j in range(tail):
            with scope(f"w6_{j}"):
                if comm:
                    for d in range(2):
                        o_fwd(d, j).wait_recv()
            with scope(f"o3_{j}"):
                cols = pl.ds(j * tw, tw)
                for b in range(B_LOC):
                    rows = pl.ds(b * SQ, SQ)
                    r = acc[rows, cols]
                    for h in range(2):
                        r += jnp.dot(ctx[DIAG, h, rows], wo[DIAG, h, :, cols], preferred_element_type=F32)
                    out_ref[b, :, cols] = r.astype(out_ref.dtype)
        with scope("wsend"):
            if comm:
                for j in range(tail):
                    for d in range(2):
                        o_fwd(d, j).wait_send()

    def fn(x, Wq, K_ext, V_ext, Wo):
        kt = jnp.transpose(K_ext, (0, 2, 3, 1)).reshape(8, 1024, 256)
        vt = jnp.transpose(V_ext, (0, 2, 3, 1)).reshape(8, 1024, 256)
        hbm = pl.BlockSpec(memory_space=pltpu.HBM)
        nq = len(wq_rows)
        return pl.pallas_call(
            body,
            out_shape=jax.ShapeDtypeStruct((B_LOC, SQ, DM), BF),
            in_specs=[hbm] * 5,
            out_specs=pl.BlockSpec(memory_space=pltpu.VMEM),
            scratch_shapes=[
                pltpu.VMEM((B_LOC, SQ, DM), F32),
                pltpu.VMEM((DM, 256), F32),
                pltpu.VMEM((256, DM), F32),
                pltpu.VMEM((4, B_LOC, 256, SQ), F32),
                pltpu.VMEM((4, B_LOC, 256, SQ), F32),
                pltpu.VMEM((TOK, DM), BF),
                pltpu.VMEM((4, 2, DM, 128), BF),
                pltpu.VMEM((4, 2, 128, DM), BF),
                pltpu.VMEM((4, 2, B_LOC, NBLK, 128, 128), BF),
                pltpu.VMEM((4, 2, B_LOC, NBLK, 128, 128), BF),
                pltpu.VMEM((4, 2, TOK, 128), BF),
                pltpu.VMEM((TOK, DM), F32),
                pltpu.SemaphoreType.DMA((nq + 10,)),
                pltpu.SemaphoreType.DMA((2, nq + 2)),
                pltpu.SemaphoreType.DMA((2, nq + 2)),
                pltpu.SemaphoreType.DMA((2, 2 + tail)),
                pltpu.SemaphoreType.DMA((2, 2 + tail)),
                pltpu.SemaphoreType.REGULAR,
            ],
            compiler_params=pltpu.CompilerParams(
                collective_id=0 if comm else None,
                disable_semaphore_checks=True,
                vmem_limit_bytes=48 * 1024 * 1024,
            ),
        )(x, Wq, kt, vt, Wo)

    return fn


def pallas_dist_sparse_attn_causalblk_htp_bs_b2_sq256_skv256_hq4_dh64_kernel(x, Wq, K_ext, V_ext, Wo):
    return make()(x, Wq, K_ext, V_ext, Wo)
```

```python
import functools
import math

import jax
import jax.numpy as jnp
from jax import lax
from jax.experimental import pallas as pl
from jax.experimental.pallas import tpu as pltpu

B_LOC, SQ, DM, DH, BLK = 2, 256, 512, 64, 64
Q_SCALE = 0.125 * math.log2(math.e)
BF, F32, I32 = jnp.bfloat16, jnp.float32, jnp.int32
MESH = pl.DeviceIdType.MESH

OWN, LEFT, RIGHT, DIAG = range(4)
WQ, WO = range(2)
PAIRS = ((OWN, 0), (OWN, 1), (LEFT, 0), (RIGHT, 1), (LEFT, 1), (RIGHT, 0), (DIAG, 0), (DIAG, 1))
UNITS = [(s, h, b) for s, h in PAIRS for b in range(B_LOC)]

NV = 32
EXP_ROWS = 48
RUNS = [range(j, min(j + 3, NV)) for j in range(0, NV, 3)]
ORDERS = ((2, 1, 0, 3, 4, 5, 6), (2, 1, 4, 3, 0, 5, 6), (2, 3, 4, 1, 6, 5, 0), (2, 3, 4, 5, 6, 1, 0))
SPREADS = (1126, 1367, 1628)
TOP_BIT = -1 << 31
SIGN_MANTISSA = ~0x7F807F80
shr = lax.shift_right_logical


def vreg(j):
    return pl.ds(8 * j, 8)


def shift(v, n):
    return v << n if n > 0 else shr(v, -n) if n < 0 else v


def exponent_max(a, b):
    return lax.bitcast_convert_type(
        jnp.maximum(lax.bitcast_convert_type(a, F32), lax.bitcast_convert_type(b, F32)), I32)


def over_sublanes(op, v, steps=(4, 2, 1)):
    for s in steps:
        v = op(v, pltpu.roll(v, s, 0))
    return v


def running_sum(v, sub):
    for s in (1, 2, 4):
        v += jnp.where(sub >= s, pltpu.roll(v, s, 0), 0)
    return v


def swap_table(order, by_rank):
    words = [sum((r ^ d) << 2 * (r if by_rank else d) for r, d in enumerate(o)) for o in ORDERS]
    table = jnp.full(order.shape, words[0], I32)
    for k in range(1, len(words)):
        table = jnp.where(order == k, words[k], table)
    return table


def swap(v, table):
    hi, lo = (shr(shr(table, i), i) for i in (shr(v, 16), v & 31))
    return v ^ (((hi << 16) | lo) & 0x00060006)


def pack_sm(a, b):
    return (a & SIGN_MANTISSA) | ((shr(b, 8) | (b << 24)) & ~SIGN_MANTISSA)


def unpack_sm(sm):
    return sm & SIGN_MANTISSA, ((sm << 8) | shr(sm, 24)) & SIGN_MANTISSA


def encode_exp(w, dst):
    sub = lax.broadcasted_iota(I32, (8, 128), 0)
    words = [w[vreg(j), :] for j in range(NV)]
    top = [exponent_max(p & 0x7F800000, (p << 16) & 0x7F800000) for p in words]
    top = shr(over_sublanes(exponent_max, functools.reduce(exponent_max, top)), 23)
    exps = [shr(p, 7) & 0x00FF00FF for p in words]
    total = functools.reduce(jnp.add, exps)
    spread = (top << 9) - over_sublanes(jnp.add, (total & 0xFFFF) + shr(total, 16))
    order = functools.reduce(jnp.add, [jnp.where(spread > t, 1, 0) for t in SPREADS])
    table = swap_table(order, by_rank=False)
    top2 = top | (top << 16)

    low = [0, 0]
    far = 0
    stream, sizes = [], []
    for run in reversed(RUNS):
        bits, size = None, 2 * len(run)
        for j in reversed(run):
            dist = top2 - exps[j]
            far |= dist
            rank = swap(dist & 0x001F001F, table)
            low[j // 16] |= shift(rank & 0x00010001, j % 16)
            for zeros in (shr(rank, 1) & 15, shr(rank, 17)):
                bits = shr(TOP_BIT if bits is None else shr(bits, 1) | TOP_BIT, zeros)
                size += zeros
        sizes.append(size)
        size = jnp.minimum(size, 31)
        spill = [bits] + [s << (32 - size) for s in stream]
        stream = ([c | shr(s, size) for c, s in zip(spill, stream)] + spill[-1:])[:5]

    extra = jnp.maximum(functools.reduce(jnp.add, sizes) - 96, 0)
    end = running_sum(extra, sub)
    misfit = functools.reduce(
        jnp.logical_or, [s > 31 for s in sizes] + [extra > 63, end > 192, (far & 0x00E000E0) != 0])
    misfit = over_sublanes(jnp.bitwise_or, jnp.where(misfit, -1, 0))

    pos = end - extra
    bit, hop = pos & 31, (shr(pos, 5) + 2 - sub) & 7
    a, b = stream[3:]
    parts = (shr(a, bit), ((a << 1) << (31 - bit)) | shr(b, bit), (b << 1) << (31 - bit))
    pool = []
    for k in range(8):
        v = 0
        for i, part in enumerate(parts):
            v = jnp.where(hop == (k - i) % 8, part, v)
        pool.append(pltpu.roll(v, k, 0) if k else v)
    head = over_sublanes(jnp.bitwise_or, (extra & 63) << (6 * shr(sub, 1)), (4, 2))
    head |= jnp.where(sub == 0, top << 24, (order << 24) | (misfit & TOP_BIT))
    for k in range(2):
        dst[vreg(k), :] = low[k]
    for k in range(3):
        dst[vreg(2 + k), :] = stream[k] | misfit
    dst[vreg(5), :] = jnp.where(sub < 2, head, functools.reduce(jnp.bitwise_or, pool))


def decode_exp(src, dst):
    sub = lax.broadcasted_iota(I32, (8, 128), 0)
    rows = [jnp.broadcast_to(src[pl.ds(40 + r, 1), :], (8, 128)) for r in range(8)]
    top = shr(rows[0], 24)
    top = (top << 23) | (top << 7)
    table = swap_table(shr(rows[1], 24) & 3, by_rank=True)
    extra = shr(jnp.where((sub & 1) == 0, rows[0], rows[1]), 6 * shr(sub, 1)) & 63
    pos = running_sum(extra, sub) - extra
    bit, row = pos & 31, shr(pos, 5)
    got = []
    for i in range(3):
        v = rows[2 + i]
        for k in range(1, 6 - i):
            v = jnp.where(row == k, rows[2 + i + k], v)
        got.append(v)
    stream = [src[vreg(2 + k), :] for k in range(3)]
    stream += [(a << bit) | shr(shr(b, 1), 31 - bit) for a, b in zip(got, got[1:])]
    low = [src[vreg(k), :] for k in range(2)]
    for k, run in enumerate(RUNS):
        bits, size = stream[0], 2 * len(run)
        for j in run:
            rank = shift(low[j // 16], -(j % 16)) & 0x00010001
            for at in (17, 1):
                zeros = lax.clz(bits)
                bits = (bits << 1) << zeros
                size += zeros
                rank |= zeros << at
            dst[vreg(j), :] = top - (swap(rank, table) << 7)
        moved = [bits] + [s << size for s in stream[1:]]
        stream = ([c | shr(s, 32 - size) for c, s in zip(moved, stream[1:])] + moved[-1:])[:len(RUNS) - 1 - k]


def misfit_words(src):
    return src[pl.ds(41, 1), :]


def low_lanes(rows):
    return lax.broadcasted_iota(I32, (rows, 128), 1) < 64


def project_q(x_ref, w):
    q = jnp.dot(pltpu.bitcast(x_ref[...], BF), w, preferred_element_type=F32)
    return [q[128 * t:128 * t + 128].astype(BF) for t in range(2)]


def split_keys(k_ref):
    k = pltpu.bitcast(k_ref[...].astype(BF).T, I32)
    first = jnp.where(low_lanes(SQ // 2), -1, 0)
    k = (k & first, k & ~first)
    return {(t, a): pltpu.bitcast(k[a][:64 * (t + 1)], BF) for t in range(2) for a in range(2)}


def softmax_t(q, k):
    out = {}
    for (t, a), keys in k.items():
        s = lax.dot_general(keys, q[t], (((1,), (1,)), ((), ())), preferred_element_type=F32)
        s = jnp.concatenate([s[:-BLK], jnp.where(low_lanes(BLK), -jnp.inf, s[-BLK:])], axis=0)
        e = jnp.exp2(s - jnp.max(s, axis=0, keepdims=True))
        out[t, a] = e.astype(BF), 1.0 / jnp.sum(e, axis=0, keepdims=True)
    return out


def context_t(p, v_ref):
    return {(t, a): jnp.dot(v_ref[pl.ds(DH * a, DH), pl.ds(0, 128 * (t + 1))].astype(BF), e,
                            preferred_element_type=F32) * inv for (t, a), (e, inv) in p.items()}


def put_context(first, second, dst):
    for t in range(2):
        dst[pl.ds(64 * t, 64), :] = pltpu.bitcast(
            jnp.concatenate([first[t], second[t]], axis=0).astype(BF).T, I32)


CUTS = {
    (WQ, 0): (0, 8, 16, 32, 64, 96, 128), (WQ, 1): (0, 8, 16, 32, 128), (WQ, 2): (0, 64, 128),
    (WO, 0): (0, 64, 128), (WO, 1): (0, 64, 128), (WO, 2): (0, 32, 64, 96, 112, 128),
}
N_COPIES = sum(len(c) for c in CUTS.values())
N_LOADS = len(CUTS[WQ, 0]) - 1 + 5 * B_LOC + 1 + 2 * (len(PAIRS) - 2)

PLAN = """
x.0 q.0 send.0.0.ex send.0.1.3 q.2 load.k.0.0 load.k.1.0 load.v.0.0 load.v.1.0 k.0 s.0 k.2 s.2 c.0
send.0.1.ex c.2 x.1 t.0 t.2 q.1 q.3 relay.1 load.k.0.1 load.k.1.1 k.1 s.1 k.3 s.3 fence load.v.0.1
load.v.1.1 wo relay.0 recv.0.0.ex c.3 send.0.2.ex send.0.2.1 send.1.0.0 decode.0.2 decode.0.3 c.1
t.1 t.3 o.0.0 o.0.1 o.0.2 o.0.3 q.4 q.5 encode.1 send.1.0.ex send.1.0.1 send.1.1.ex send.1.1.0
load.k.2 load.v.2 load.k.3 load.v.3 recv.0.1.ex decode.0.4 q.6 k.4 decode.0.5 load.k.4 s.4 q.7 k.5
s.5 c.4 c.5 t.4 k.6 recv.0.1.3 s.6 t.5 k.7 s.7 load.v.4 load.k.5 load.v.5 recv.0.1.0 recv.0.1.1
recv.0.1.2 q.8 c.6 t.6 c.7 t.7 q.9 k.8 s.8 q.10 c.8 k.9 q.11 k.11 send.1.1.1 load.k.6 t.8
recv.0.2.ex decode.0.6 s.9 decode.0.7 k.10 s.10 c.9 t.9 load.v.6 load.k.7 load.v.7 recv.0.2.0
recv.0.2.1 s.11 recv.1.0.0 recv.1.0.ex c.11 c.10 send.1.2.ex t.10 q.12 q.13 k.12 send.1.2.0 t.11
send.1.2.1 decode.1.2 decode.1.3 s.12 q.14 k.13 s.13 c.12 q.15 recv.1.0.1 send.1.2.2 send.1.2.3
send.1.2.4 recv.1.1.ex k.14 decode.1.4 s.14 o.1.3 c.13 k.15 s.15 decode.1.5 c.14 o.1.1 t.12 t.14
c.15 t.13 t.15 o.1.0 o.1.2 recv.1.1.0 o.2.0 recv.1.1.1 o.2.1 fence recv.1.2.ex decode.1.6
decode.1.7 o.2.3 recv.1.2.0 o.3.0 o.2.2 sent.1.0 sent.1.1 recv.1.2.1 o.3.1 sent.0.0 sent.0.1
sent.0.2 check recv.1.2.2 o.3.2 recv.1.2.3 o.3.3.0 sent.1.2.ex.0.1.2 recv.1.2.4 o.3.3.1
sent.1.2.3.4
"""


def kernel_body(x_hbm, wq_hbm, k_hbm, v_hbm, wo_hbm, out_ref,
                x_f, wq_f, wo_f, k_f, v_f, xb, w_own, sm, ex, eb, ctx, acc, raw,
                ld_sem, send_sem, recv_sem, raw_send, raw_recv, go_sem, fence_sem):
    loads = {}

    def start_load(name, src, dst):
        loads[name] = pltpu.make_async_copy(src, dst, ld_sem.at[len(loads)])
        loads[name].start()

    wq_rows = [pl.ds(4 * a, 4 * (b - a)) for a, b in zip(CUTS[WQ, 0], CUTS[WQ, 0][1:])]
    for i, rows in enumerate(wq_rows):
        start_load(("wq", i), wq_hbm.at[rows], wq_f.at[rows])

    me = lax.axis_index("i")
    chip = (me, (me + 3) & 3, (me + 1) & 3, (me + 2) & 3)
    odd = (me & 1) == 1
    barrier = pltpu.get_barrier_semaphore()

    def greet(sem):
        for side in (LEFT, RIGHT):
            pl.semaphore_signal(sem, inc=1, device_id=(chip[side],), device_id_type=MESH)

    pl.when(me != 2)(lambda: greet(barrier))

    def head_rows(slot, h):
        return pl.ds(pl.multiple_of(chip[slot] * 256 + h * 128, 128), 128)

    for b in range(B_LOC):
        start_load(("x", b), x_hbm.at[b], x_f.at[b])
        for name, hbm, dst in (("k", k_hbm, k_f), ("v", v_hbm, v_f)):
            for h in range(2):
                start_load((name, h, b), hbm.at[me * B_LOC + b, head_rows(OWN, h)], dst.at[OWN, h, b])
    start_load("wo", wo_hbm, wo_f)
    for p in range(2, len(PAIRS)):
        for name, hbm, dst in (("k", k_hbm, k_f), ("v", v_hbm, v_f)):
            start_load((name, p), hbm.at[pl.ds(me * B_LOC, B_LOC), head_rows(*PAIRS[p])], dst.at[PAIRS[p]])

    def remote(src, dst, send_on, recv_on, d):
        return pltpu.make_async_remote_copy(
            src, dst, send_on, recv_on, device_id=(chip[(RIGHT, LEFT)[d]],), device_id_type=MESH)

    sem_of = {}

    def rdma(m, hop, part, d):
        n = sem_of.setdefault((m, hop, part), len(sem_of))
        h = 1 - d if hop == 1 else d
        near = (LEFT, RIGHT)[d]
        here, there = (near, DIAG) if hop == 2 else (OWN, near)
        if part == "ex":
            src, dst = ex.at[m, here, h], ex.at[m, there, h]
        else:
            rows = pl.ds(CUTS[m, hop][part], CUTS[m, hop][part + 1] - CUTS[m, hop][part])
            src, dst = sm.at[m, here, h, rows], sm.at[m, there, h, rows]
        return remote(src, dst, send_sem.at[d, n], recv_sem.at[d, n], d)

    def put_own(m, h, row, w):
        p = pltpu.bitcast(w.astype(BF), I32)
        w_own[m, h, pl.ds(row, p.shape[0]), :] = p
        for r in range(0, p.shape[0], 16):
            sm[m, OWN, h, pl.ds((row + r) // 2, 8), :] = pack_sm(p[r:r + 8], p[r + 8:r + 16])

    def encode(m):
        for h in range(2):
            encode_exp(w_own.at[m, h], ex.at[m, OWN, h])

    def send_wq_rows(i, d):
        rdma(WQ, 0, i, d).start()
        if i < len(CUTS[WQ, 1]) - 2:
            rdma(WQ, 1, i, d).start()

    pl.when(odd)(lambda: pl.semaphore_wait(barrier, 1))

    @pl.when(me == 2)
    def _():
        pl.semaphore_wait(barrier, 2)
        greet(go_sem)

    known = (me >= 2, jnp.logical_or(me == 1, me == 2))
    for i, rows in enumerate(wq_rows):
        loads["wq", i].wait()
        for h in range(2):
            put_own(WQ, h, rows.start // 2, wq_f[rows, pl.ds(128 * h, 128)])
        for d in range(2):
            pl.when(known[d])(functools.partial(send_wq_rows, i, d))
    encode(WQ)
    pl.when(me == 0)(lambda: pl.semaphore_wait(barrier, 2))
    pl.when(odd)(lambda: pl.semaphore_wait(go_sem, 1))
    for d in range(2):
        @pl.when(jnp.logical_not(known[d]))
        def _():
            for i in range(len(wq_rows)):
                send_wq_rows(i, d)

    def weights(m, slot, h, j0, nj):
        if slot == OWN:
            return [w_own[m, h, pl.ds(8 * j0, 8 * nj), :]]
        return [half | eb[m, slot, h, vreg(2 * n + i), :]
                for n in range(j0 // 2, (j0 + nj) // 2)
                for i, half in enumerate(unpack_sm(sm[m, slot, h, vreg(n), :]))]

    def as_bf16(words):
        return pltpu.bitcast(jnp.concatenate(words, axis=0), BF)

    live = {}

    def send(m, hop, part):
        for d in range(2):
            rdma(m, hop, part, d).start()

    def recv(m, hop, part):
        for d in range(2):
            rdma(m, hop, part, d).wait_recv()

    def sent(m, hop, *parts):
        for part in parts or ("ex", *range(len(CUTS[m, hop]) - 1)):
            for d in range(2):
                rdma(m, hop, part, d).wait_send()

    def relay(others):
        @pl.when((me != 0) if others else (me == 0))
        def _():
            for i in range(len(wq_rows)):
                recv(WQ, 0, i)
            send(WQ, 2, 0)

    def fence():
        pl.semaphore_signal(fence_sem, inc=1)
        pl.semaphore_wait(fence_sem, 1)

    def load(*name):
        loads[name].wait()

    def x(b):
        load("x", b)
        xb[b] = pltpu.bitcast((x_f[b] * Q_SCALE).astype(BF), I32)

    def wo():
        loads["wo"].wait()
        for h in range(2):
            for j in range(4):
                put_own(WO, h, 64 * j, wo_f[pl.ds(128 * h, 128), pl.ds(128 * j, 128)])

    def decode(m, p):
        decode_exp(ex.at[(m, *PAIRS[p])], eb.at[(m, *PAIRS[p])])

    def q(i):
        slot, h, b = UNITS[i]
        if ("w", slot, h) not in live:
            live["w", slot, h] = as_bf16(weights(WQ, slot, h, 0, NV))
        live["q", i] = project_q(xb.at[b], live["w", slot, h])

    def k(i):
        live["k", i] = split_keys(k_f.at[UNITS[i]])

    def s(i):
        live["p", i] = softmax_t(live["q", i], live["k", i])

    def c(i):
        live["c", i] = context_t(live["p", i], v_f.at[UNITS[i]])

    def t(i):
        slot, h, b = UNITS[i]
        heads = [(UNITS.index((DIAG, n, b)), h) if slot == DIAG else (i, n) for n in range(2)]
        put_context(*[[live["c", u][tile, a] for tile in range(2)] for u, a in heads], ctx.at[UNITS[i]])

    def o(g, j, *which):
        terms = []
        for n in which or range(2):
            slot, h = PAIRS[2 * g + n]
            terms.append((slot, h, as_bf16(
                weights(WO, slot, h, 8 * j, 8) if slot != DIAG else
                weights(WO, slot, 0, 8 * j + 4 * h, 4) + weights(WO, slot, 1, 8 * j + 4 * h, 4))))
        before = live.get(("o", j), 0)
        live["o", j] = before + len(terms)
        cols, size = pl.ds(128 * j, 128), 128 * len(terms)
        for b in range(B_LOC):
            for r in range(0, SQ, size):
                y = functools.reduce(jnp.add, [
                    jnp.dot(pltpu.bitcast(ctx[slot, h, b, pl.ds(r // 2, size // 2), :], BF), w,
                            preferred_element_type=F32) for slot, h, w in terms])
                if before:
                    y += acc[b, pl.ds(r, size), cols]
                if live["o", j] < len(PAIRS):
                    acc[b, pl.ds(r, size), cols] = y
                else:
                    out_ref[b, pl.ds(r, size), cols] = y.astype(out_ref.dtype)

    def check():
        words = [misfit_words(ex.at[m, slot, h]) for m in (WQ, WO) for slot, h in PAIRS]
        live["misfit"] = jnp.max(jnp.where(functools.reduce(jnp.bitwise_or, words) < 0, 1.0, 0.0)) > 0.0

    steps = dict(send=send, recv=recv, sent=sent, relay=relay, fence=fence, load=load, x=x, wo=wo,
                 encode=encode, decode=decode, q=q, k=k, s=s, c=c, t=t, o=o, check=check)
    for step in PLAN.split():
        name, *args = step.split(".")
        steps[name](*(int(a) if a.isdigit() else a for a in args))

    @pl.when(live["misfit"])
    def _():
        for hop in range(2):
            copies = [remote(*((raw.at[near, d], raw.at[DIAG, d]) if hop else (w_own, raw.at[near])),
                             raw_send.at[hop, d], raw_recv.at[hop, d], d)
                      for d, near in enumerate((LEFT, RIGHT))]
            for copy in copies:
                copy.start()
            for copy in copies:
                copy.wait()
        raw[OWN] = w_own[...]
        acc[...] = jnp.zeros(acc.shape, F32)

        @pl.loop(0, len(UNITS))
        def _(i):
            slot, h, b = i >> 2, (i >> 1) & 1, i & 1
            query = project_q(xb.at[b], pltpu.bitcast(raw[slot, WQ, h], BF))
            heads = context_t(softmax_t(query, split_keys(k_f.at[slot, h, b])), v_f.at[slot, h, b])
            put_context(*[[heads[tile, a] for tile in range(2)] for a in range(2)], ctx.at[slot, h, b])
            for j in range(4):
                acc[b, :, pl.ds(128 * j, 128)] += jnp.dot(
                    pltpu.bitcast(ctx[slot, h, b], BF),
                    pltpu.bitcast(raw[slot, WO, h, pl.ds(64 * j, 64), :], BF), preferred_element_type=F32)

        out_ref[...] = acc[...].astype(out_ref.dtype)


def pallas_dist_sparse_attn_causalblk_htp_bs_b2_sq256_skv256_hq4_dh64_kernel(
    x: jax.Array,
    Wq: jax.Array,
    K_ext: jax.Array,
    V_ext: jax.Array,
    Wo: jax.Array,
):
    kt = jnp.transpose(K_ext, (0, 2, 3, 1)).reshape(8, 16 * DH, SQ)
    vt = jnp.transpose(V_ext, (0, 2, 3, 1)).reshape(8, 16 * DH, SQ)
    return pl.pallas_call(
        kernel_body,
        out_shape=jax.ShapeDtypeStruct((B_LOC, SQ, DM), BF),
        in_specs=[pl.BlockSpec(memory_space=pltpu.HBM)] * 5,
        out_specs=pl.BlockSpec(memory_space=pltpu.VMEM),
        scratch_shapes=[
            pltpu.VMEM((B_LOC, SQ, DM), F32),
            pltpu.VMEM((DM, 256), F32),
            pltpu.VMEM((256, DM), F32),
            pltpu.VMEM((4, 2, B_LOC, 128, SQ), F32),
            pltpu.VMEM((4, 2, B_LOC, 128, SQ), F32),
            pltpu.VMEM((B_LOC, SQ // 2, DM), I32),
            pltpu.VMEM((2, 2, 8 * NV, 128), I32),
            pltpu.VMEM((2, 4, 2, 4 * NV, 128), I32),
            pltpu.VMEM((2, 4, 2, EXP_ROWS, 128), I32),
            pltpu.VMEM((2, 4, 2, 8 * NV, 128), I32),
            pltpu.VMEM((4, 2, B_LOC, SQ // 2, 128), I32),
            pltpu.VMEM((B_LOC, SQ, DM), F32),
            pltpu.VMEM((4, 2, 2, 8 * NV, 128), I32),
            pltpu.SemaphoreType.DMA((N_LOADS,)),
            pltpu.SemaphoreType.DMA((2, N_COPIES)),
            pltpu.SemaphoreType.DMA((2, N_COPIES)),
            pltpu.SemaphoreType.DMA((2, 2)),
            pltpu.SemaphoreType.DMA((2, 2)),
            pltpu.SemaphoreType.REGULAR,
            pltpu.SemaphoreType.REGULAR,
        ],
        compiler_params=pltpu.CompilerParams(
            collective_id=0,
            disable_semaphore_checks=True,
            vmem_limit_bytes=48 * 1024 * 1024,
            flags={"XLA_TPU_RESCHEDULE_DMA_DONES": True},
        ),
    )(x, Wq, kt, vt, Wo)
```

```python
import functools
import math

import jax
import jax.numpy as jnp
from jax import lax
from jax.experimental import pallas as pl
from jax.experimental.pallas import tpu as pltpu

B_LOC, SQ, DM, DH, BLK = 2, 256, 512, 64, 64
Q_SCALE = 0.125 * math.log2(math.e)
BF, F32, I32 = jnp.bfloat16, jnp.float32, jnp.int32
MESH = pl.DeviceIdType.MESH

OWN, LEFT, RIGHT, DIAG = range(4)
WQ, WO = range(2)
PAIRS = ((OWN, 0), (OWN, 1), (LEFT, 0), (RIGHT, 1), (LEFT, 1), (RIGHT, 0), (DIAG, 0), (DIAG, 1))
UNITS = [(s, h, b) for s, h in PAIRS for b in range(B_LOC)]

NV = 32
EXP_ROWS = 48
RUNS = [range(j, min(j + 3, NV)) for j in range(0, NV, 3)]
ORDERS = ((2, 1, 0, 3, 4, 5, 6), (2, 1, 4, 3, 0, 5, 6), (2, 3, 4, 1, 6, 5, 0), (2, 3, 4, 5, 6, 1, 0))
LEVELS = (171.0, 125.0, 86.0)
TOP_BIT = -1 << 31
SIGN_MANTISSA = ~0x7F807F80
shr = lax.shift_right_logical


def vreg(j):
    return pl.ds(8 * j, 8)


def shift(v, n):
    return v << n if n > 0 else shr(v, -n) if n < 0 else v


def over_sublanes(op, v, steps=(4, 2, 1)):
    for s in steps:
        v = op(v, pltpu.roll(v, s, 0))
    return v


def running_sum(v, sub):
    for s in (1, 2, 4):
        v += jnp.where(sub >= s, pltpu.roll(v, s, 0), 0)
    return v


def swap_table(order, by_rank):
    words = [sum((r ^ d) << 2 * (r if by_rank else d) for r, d in enumerate(o)) for o in ORDERS]
    table = jnp.full(order.shape, words[0], I32)
    for k in range(1, len(words)):
        table = jnp.where(order == k, words[k], table)
    return table


def swap(v, table):
    hi, lo = (shr(shr(table, i), i) for i in (shr(v, 16), v & 31))
    return v ^ (((hi << 16) | lo) & 0x00060006)


def pack_sm(a, b):
    return (a & SIGN_MANTISSA) | ((shr(b, 8) | (b << 24)) & ~SIGN_MANTISSA)


def unpack_sm(sm):
    return sm & SIGN_MANTISSA, ((sm << 8) | shr(sm, 24)) & SIGN_MANTISSA


def encode_exp(w, dst):
    sub = lax.broadcasted_iota(I32, (8, 128), 0)
    words = [w[vreg(j), :] for j in range(NV)]
    powers = [[lax.bitcast_convert_type(v & 0x7F800000, F32) for v in (p, p << 16)] for p in words]
    top, total = (over_sublanes(op, functools.reduce(op, [op(*pair) for pair in powers]))
                  for op in (jnp.maximum, jnp.add))
    order = functools.reduce(jnp.add, [jnp.where(total < level * top, 1, 0) for level in LEVELS])
    top = shr(lax.bitcast_convert_type(top, I32), 23)
    table = swap_table(order, by_rank=False)
    top2 = top | (top << 16)

    low = [0, 0]
    far = 0
    stream, sizes = [], []
    for run in reversed(RUNS):
        bits, size = None, 2 * len(run)
        for j in reversed(run):
            dist = top2 - (shr(words[j], 7) & 0x00FF00FF)
            far |= dist
            rank = swap(dist & 0x001F001F, table)
            low[j // 16] |= shift(rank & 0x00010001, j % 16)
            for zeros in (shr(rank, 1) & 15, shr(rank, 17)):
                bits = (1 if bits is None else (bits << 1) | 1) << zeros
                size += zeros
        sizes.append(size)
        size = jnp.minimum(size, 31)
        spill = [bits] + [shr(s, 32 - size) for s in stream]
        stream = ([c | (s << size) for c, s in zip(spill, stream)] + spill[-1:])[:5]

    extra = jnp.maximum(functools.reduce(jnp.add, sizes) - 96, 0)
    end = running_sum(extra, sub)
    misfit = functools.reduce(
        jnp.logical_or, [s > 31 for s in sizes] + [extra > 63, end > 192, (far & 0x00E000E0) != 0])
    misfit = over_sublanes(jnp.bitwise_or, jnp.where(misfit, -1, 0))

    pos = end - extra
    bit, hop = pos & 31, (shr(pos, 5) + 2 - sub) & 7
    a, b = stream[3:]
    parts = (a << bit, shr(shr(a, 1), 31 - bit) | (b << bit), shr(shr(b, 1), 31 - bit))
    pool = []
    for k in range(8):
        v = 0
        for i, part in enumerate(parts):
            v = jnp.where(hop == (k - i) % 8, part, v)
        pool.append(pltpu.roll(v, k, 0) if k else v)
    head = over_sublanes(jnp.bitwise_or, (extra & 63) << (6 * shr(sub, 1)), (4, 2))
    head |= jnp.where(sub == 0, top << 24, (order << 24) | (misfit & TOP_BIT))
    for k in range(2):
        dst[vreg(k), :] = low[k]
    for k in range(3):
        dst[vreg(2 + k), :] = stream[k] | misfit
    dst[vreg(5), :] = jnp.where(sub < 2, head, functools.reduce(jnp.bitwise_or, pool))


def decode_exp(src, dst):
    sub = lax.broadcasted_iota(I32, (8, 128), 0)
    rows = [jnp.broadcast_to(src[pl.ds(40 + r, 1), :], (8, 128)) for r in range(8)]
    top = shr(rows[0], 24)
    top = (top << 23) | (top << 7)
    table = swap_table(shr(rows[1], 24) & 3, by_rank=True)
    extra = shr(jnp.where((sub & 1) == 0, rows[0], rows[1]), 6 * shr(sub, 1)) & 63
    pos = running_sum(extra, sub) - extra
    bit, row = pos & 31, shr(pos, 5)
    got = []
    for i in range(3):
        v = rows[2 + i]
        for k in range(1, 6 - i):
            v = jnp.where(row == k, rows[2 + i + k], v)
        got.append(v)
    stream = [src[vreg(2 + k), :] for k in range(3)]
    stream += [shr(a, bit) | ((b << 1) << (31 - bit)) for a, b in zip(got, got[1:])]
    low = [src[vreg(k), :] for k in range(2)]
    for k, run in enumerate(RUNS):
        bits, last = stream[0], 126 << 23
        for j in run:
            rank = (shift(low[j // 16], -(j % 16)) & 0x00010001) - 0x00020002
            for at in (17, 1):
                rest = bits & (bits - 1)
                stop = lax.bitcast_convert_type((bits ^ rest).astype(F32), I32)
                rank += shr(stop - last, 23 - at)
                bits, last = rest, stop
            dst[vreg(j), :] = top - (swap(rank, table) << 7)
        size = shr(last, 23) - 126
        moved = [shr(s, size) for s in stream]
        stream = ([c | (s << (32 - size)) for c, s in zip(moved, stream[1:])] + moved[-1:])[:len(RUNS) - 1 - k]


def misfit_words(src):
    return src[pl.ds(41, 1), :]


def low_lanes(rows):
    return lax.broadcasted_iota(I32, (rows, 128), 1) < 64


def project_q(x_ref, w):
    q = jnp.dot(pltpu.bitcast(x_ref[...], BF), w, preferred_element_type=F32)
    return [q[128 * t:128 * t + 128].astype(BF) for t in range(2)]


def split_keys(k_ref):
    k = pltpu.bitcast(k_ref[...].astype(BF).T, I32)
    first = jnp.where(low_lanes(SQ // 2), -1, 0)
    k = (k & first, k & ~first)
    return {(t, a): pltpu.bitcast(k[a][:64 * (t + 1)], BF) for t in range(2) for a in range(2)}


def softmax_t(q, k):
    out = {}
    for (t, a), keys in k.items():
        s = lax.dot_general(keys, q[t], (((1,), (1,)), ((), ())), preferred_element_type=F32)
        s = jnp.concatenate([s[:-BLK], jnp.where(low_lanes(BLK), -jnp.inf, s[-BLK:])], axis=0)
        e = jnp.exp2(s - jnp.max(s, axis=0, keepdims=True))
        out[t, a] = e.astype(BF), 1.0 / jnp.sum(e, axis=0, keepdims=True)
    return out


def context_t(p, v_ref):
    return {(t, a): jnp.dot(v_ref[pl.ds(DH * a, DH), pl.ds(0, 128 * (t + 1))].astype(BF), e,
                            preferred_element_type=F32) * inv for (t, a), (e, inv) in p.items()}


def put_context(first, second, dst):
    for t in range(2):
        dst[pl.ds(64 * t, 64), :] = pltpu.bitcast(
            jnp.concatenate([first[t], second[t]], axis=0).astype(BF).T, I32)


CUTS = {
    (WQ, 0): (0, 8, 16, 32, 64, 96, 128), (WQ, 1): (0, 8, 16, 32, 128), (WQ, 2): (0, 64, 128),
    (WO, 0): (0, 64, 128), (WO, 1): (0, 64, 128), (WO, 2): (0, 32, 64, 96, 112, 128),
}
N_COPIES = sum(2 if m == WQ else len(c) for (m, _), c in CUTS.items())
N_LOADS = len(CUTS[WQ, 0]) + 5 * B_LOC + 1 + 2 * (len(PAIRS) - 2)

PLAN = """
x.0 q.0 send.0.0.ex q.2 send.0.1.ex load.k.0.0 load.k.1.0 load.v.0.0 k.0 s.0 k.2 s.2 c.0 load.v.1.0
c.2 send.0.1.3 x.1 t.0 t.2 q.1 q.3 load.k.0.1 load.k.1.1 k.1 relay.1 s.1 k.3 s.3 load.v.0.1
load.v.1.1 fence wo recv.0.0.ex c.3 send.0.2.ex relay.0 send.0.2.1 send.1.0.0 decode.0.3 c.1 t.1
decode.0.2 t.3 o.0.1 o.0.2 o.0.0 o.0.3 q.4 q.5 encode.1 send.1.0.ex send.1.1.ex load.k.3 send.1.0.1
send.1.1.0 q.6 load.v.3 recv.0.1.ex load.k.2 load.v.2 k.5 decode.0.4 k.4 s.4 s.5 decode.0.5 load.k.4
q.7 c.4 c.5 t.4 k.6 recv.0.1.sm s.6 t.5 k.7 s.7 load.k.5 q.8 c.6 load.v.5 c.7 load.v.4 t.7 t.6 q.9
k.8 s.8 q.10 send.1.1.1 k.9 c.8 k.11 q.11 recv.0.2.ex s.9 decode.0.6 decode.0.7 k.10 s.10 load.v.7
s.11 recv.1.0.0 t.8 recv.1.0.ex c.9 t.9 decode.1.2 load.v.6 load.k.7 recv.0.2.sm c.11 c.10
send.1.2.ex load.k.6 t.10 q.12 q.13 k.12 send.1.2.0 q.14 k.13 recv.1.1.ex s.12 q.15 s.13 send.1.2.1
k.14 t.11 c.12 decode.1.3 s.14 recv.1.0.1 send.1.2.2 decode.1.4 send.1.2.3 send.1.2.4 o.1.3 sent.0.0
decode.1.5 sent.0.2 c.13 k.15 c.14 t.12 t.14 sent.1.0 s.15 o.1.0 o.1.1 c.15 sent.0.1 t.13 o.1.2
sent.1.1 recv.1.1.1 t.15 recv.1.1.0 o.2.0 o.2.1 o.2.2 recv.1.2.ex decode.1.6 check fence decode.1.7
recv.1.2.0 o.2.3 o.3.0.2.0.240 recv.1.2.1 o.3.1.2.0.240 o.3.0.2.240.256 sent.1.2 recv.1.2.2
o.3.2.2.0.240 o.3.1.2.240.256 recv.1.2.3 o.3.3.0 o.3.2.2.240.256 recv.1.2.4 o.3.3.1
"""


def kernel_body(x_hbm, wq_hbm, k_hbm, v_hbm, wo_hbm, out_ref,
                x_f, wq_f, wo_f, k_f, v_f, xb, w_own, sm, ex, eb, ctx, acc, raw,
                ld_sem, send_sem, recv_sem, raw_send, raw_recv, go_sem, fence_sem):
    loads = {}

    def start_load(name, src, dst):
        loads[name] = pltpu.make_async_copy(src, dst, ld_sem.at[len(loads)])
        loads[name].start()

    wq_rows = [pl.ds(4 * a, 4 * (b - a)) for a, b in zip(CUTS[WQ, 0], CUTS[WQ, 0][1:])]
    wq_parts = [(0, (0,)), (0, (1,))] + [(i, (0, 1)) for i in range(1, len(wq_rows))]
    for i, halves in wq_parts:
        at = wq_rows[i], pl.ds(128 * halves[0], 128 * len(halves))
        start_load(("wq", i, halves), wq_hbm.at[at], wq_f.at[at])

    me = lax.axis_index("i")
    chip = (me, (me + 3) & 3, (me + 1) & 3, (me + 2) & 3)
    odd = (me & 1) == 1
    barrier = pltpu.get_barrier_semaphore()

    def greet(sem):
        for side in (LEFT, RIGHT):
            pl.semaphore_signal(sem, inc=1, device_id=(chip[side],), device_id_type=MESH)

    pl.when(me != 2)(lambda: greet(barrier))

    def head_rows(slot, h):
        return pl.ds(pl.multiple_of(chip[slot] * 256 + h * 128, 128), 128)

    for b in range(B_LOC):
        start_load(("x", b), x_hbm.at[b], x_f.at[b])
        for name, hbm, dst in (("k", k_hbm, k_f), ("v", v_hbm, v_f)):
            for h in range(2):
                start_load((name, h, b), hbm.at[me * B_LOC + b, head_rows(OWN, h)], dst.at[OWN, h, b])
    start_load("wo", wo_hbm, wo_f)
    for p in range(2, len(PAIRS)):
        for name, hbm, dst in (("k", k_hbm, k_f), ("v", v_hbm, v_f)):
            start_load((name, p), hbm.at[pl.ds(me * B_LOC, B_LOC), head_rows(*PAIRS[p])], dst.at[PAIRS[p]])

    def remote(src, dst, send_on, recv_on, d):
        return pltpu.make_async_remote_copy(
            src, dst, send_on, recv_on, device_id=(chip[(RIGHT, LEFT)[d]],), device_id_type=MESH)

    sem_of = {}

    def rdma(m, hop, part, d):
        n = sem_of.setdefault((m, hop, "sm" if m == WQ and part != "ex" else part), len(sem_of))
        h = 1 - d if hop == 1 else d
        near = (LEFT, RIGHT)[d]
        here, there = (near, DIAG) if hop == 2 else (OWN, near)
        if part == "ex":
            buf, rows = ex, pl.ds(0, EXP_ROWS)
        elif part == "sm":
            buf, rows = sm, pl.ds(0, 4 * NV)
        else:
            buf, rows = sm, pl.ds(CUTS[m, hop][part], CUTS[m, hop][part + 1] - CUTS[m, hop][part])
        src, dst = buf.at[m, here, h, rows], buf.at[m, there, h, rows]
        return remote(src, dst, send_sem.at[d, n], recv_sem.at[d, n], d)

    def put_own(m, h, row, w):
        p = pltpu.bitcast(w.astype(BF), I32)
        w_own[m, h, pl.ds(row, p.shape[0]), :] = p
        for r in range(0, p.shape[0], 16):
            sm[m, OWN, h, pl.ds((row + r) // 2, 8), :] = pack_sm(p[r:r + 8], p[r + 8:r + 16])

    def encode(m):
        for h in range(2):
            encode_exp(w_own.at[m, h], ex.at[m, OWN, h])

    def send_wq_rows(i, halves, d):
        for h in halves:
            if h == d or i < len(CUTS[WQ, 1]) - 2:
                rdma(WQ, int(h != d), i, d).start()

    pl.when(odd)(lambda: pl.semaphore_wait(barrier, 1))

    @pl.when(me == 2)
    def _():
        pl.semaphore_wait(barrier, 2)
        greet(go_sem)

    known = (me >= 2, jnp.logical_or(me == 1, me == 2))
    for i, halves in wq_parts:
        loads["wq", i, halves].wait()
        for h in halves:
            put_own(WQ, h, wq_rows[i].start // 2, wq_f[wq_rows[i], pl.ds(128 * h, 128)])
        for d in range(2):
            pl.when(known[d])(functools.partial(send_wq_rows, i, halves, d))
    encode(WQ)
    pl.when(me == 0)(lambda: pl.semaphore_wait(barrier, 2))
    pl.when(odd)(lambda: pl.semaphore_wait(go_sem, 1))
    for d in range(2):
        @pl.when(jnp.logical_not(known[d]))
        def _():
            for i, halves in wq_parts:
                send_wq_rows(i, halves, d)

    def weights(m, slot, h, j0, nj):
        if slot == OWN:
            return [w_own[m, h, pl.ds(8 * j0, 8 * nj), :]]
        return [half | eb[m, slot, h, vreg(2 * n + i), :]
                for n in range(j0 // 2, (j0 + nj) // 2)
                for i, half in enumerate(unpack_sm(sm[m, slot, h, vreg(n), :]))]

    def as_bf16(words):
        return pltpu.bitcast(jnp.concatenate(words, axis=0), BF)

    live = {}

    def send(m, hop, part):
        for d in range(2):
            rdma(m, hop, part, d).start()

    def recv(m, hop, part):
        for d in range(2):
            rdma(m, hop, part, d).wait_recv()

    def sent(m, hop):
        for part in ("ex", "sm") if m == WQ else ("ex", *range(len(CUTS[m, hop]) - 1)):
            for d in range(2):
                rdma(m, hop, part, d).wait_send()

    def relay(others):
        @pl.when((me != 0) if others else (me == 0))
        def _():
            recv(WQ, 0, "sm")
            send(WQ, 2, 0)

    def fence():
        pl.semaphore_signal(fence_sem, inc=1)
        pl.semaphore_wait(fence_sem, 1)

    def load(*name):
        loads[name].wait()

    def x(b):
        load("x", b)
        xb[b] = pltpu.bitcast((x_f[b] * Q_SCALE).astype(BF), I32)

    def wo():
        loads["wo"].wait()
        for h in range(2):
            for j in range(4):
                put_own(WO, h, 64 * j, wo_f[pl.ds(128 * h, 128), pl.ds(128 * j, 128)])

    def decode(m, p):
        decode_exp(ex.at[(m, *PAIRS[p])], eb.at[(m, *PAIRS[p])])

    def q(i):
        slot, h, b = UNITS[i]
        if ("w", slot, h) not in live:
            live["w", slot, h] = as_bf16(weights(WQ, slot, h, 0, NV))
        live["q", i] = project_q(xb.at[b], live["w", slot, h])

    def k(i):
        live["k", i] = split_keys(k_f.at[UNITS[i]])

    def s(i):
        live["p", i] = softmax_t(live["q", i], live["k", i])

    def c(i):
        live["c", i] = context_t(live["p", i], v_f.at[UNITS[i]])

    def t(i):
        slot, h, b = UNITS[i]
        heads = [(UNITS.index((DIAG, n, b)), h) if slot == DIAG else (i, n) for n in range(2)]
        put_context(*[[live["c", u][tile, a] for tile in range(2)] for u, a in heads], ctx.at[UNITS[i]])

    def o(g, j, which=2, first=0, last=SQ):
        terms = []
        for n in range(2) if which == 2 else (which,):
            slot, h = PAIRS[2 * g + n]
            terms.append((slot, h, as_bf16(
                weights(WO, slot, h, 8 * j, 8) if slot != DIAG else
                weights(WO, slot, 0, 8 * j + 4 * h, 4) + weights(WO, slot, 1, 8 * j + 4 * h, 4))))
        added = live.setdefault(("o", j), [0] * SQ)
        (before,) = set(added[first:last])
        added[first:last] = [before + len(terms)] * (last - first)
        cols, size = pl.ds(128 * j, 128), (last - first) * len(terms) // 2
        for b in range(B_LOC):
            for r in range(first, last, size):
                y = functools.reduce(jnp.add, [
                    jnp.dot(pltpu.bitcast(ctx[slot, h, b, pl.ds(r // 2, size // 2), :], BF), w,
                            preferred_element_type=F32) for slot, h, w in terms])
                if before:
                    y += acc[b, pl.ds(r, size), cols]
                if added[first] < len(PAIRS):
                    acc[b, pl.ds(r, size), cols] = y
                else:
                    out_ref[b, pl.ds(r, size), cols] = y.astype(out_ref.dtype)

    def check():
        words = [misfit_words(ex.at[m, slot, h]) for m in (WQ, WO) for slot, h in PAIRS]
        live["misfit"] = jnp.max(jnp.where(functools.reduce(jnp.bitwise_or, words) < 0, 1.0, 0.0)) > 0.0

    steps = dict(send=send, recv=recv, sent=sent, relay=relay, fence=fence, load=load, x=x, wo=wo,
                 encode=encode, decode=decode, q=q, k=k, s=s, c=c, t=t, o=o, check=check)
    for step in PLAN.split():
        name, *args = step.split(".")
        steps[name](*(int(a) if a.isdigit() else a for a in args))
    assert all(set(live["o", j]) == {len(PAIRS)} for j in range(4))

    @pl.when(live["misfit"])
    def _():
        for hop in range(2):
            copies = [remote(*((raw.at[near, d], raw.at[DIAG, d]) if hop else (w_own, raw.at[near])),
                             raw_send.at[hop, d], raw_recv.at[hop, d], d)
                      for d, near in enumerate((LEFT, RIGHT))]
            for copy in copies:
                copy.start()
            for copy in copies:
                copy.wait()
        raw[OWN] = w_own[...]
        acc[...] = jnp.zeros(acc.shape, F32)

        @pl.loop(0, len(UNITS))
        def _(i):
            slot, h, b = i >> 2, (i >> 1) & 1, i & 1
            query = project_q(xb.at[b], pltpu.bitcast(raw[slot, WQ, h], BF))
            heads = context_t(softmax_t(query, split_keys(k_f.at[slot, h, b])), v_f.at[slot, h, b])
            put_context(*[[heads[tile, a] for tile in range(2)] for a in range(2)], ctx.at[slot, h, b])
            for j in range(4):
                acc[b, :, pl.ds(128 * j, 128)] += jnp.dot(
                    pltpu.bitcast(ctx[slot, h, b], BF),
                    pltpu.bitcast(raw[slot, WO, h, pl.ds(64 * j, 64), :], BF), preferred_element_type=F32)

        out_ref[...] = acc[...].astype(out_ref.dtype)


def pallas_dist_sparse_attn_causalblk_htp_bs_b2_sq256_skv256_hq4_dh64_kernel(
    x: jax.Array,
    Wq: jax.Array,
    K_ext: jax.Array,
    V_ext: jax.Array,
    Wo: jax.Array,
):
    kt = jnp.transpose(K_ext, (0, 2, 3, 1)).reshape(8, 16 * DH, SQ)
    vt = jnp.transpose(V_ext, (0, 2, 3, 1)).reshape(8, 16 * DH, SQ)
    return pl.pallas_call(
        kernel_body,
        out_shape=jax.ShapeDtypeStruct((B_LOC, SQ, DM), BF),
        in_specs=[pl.BlockSpec(memory_space=pltpu.HBM)] * 5,
        out_specs=pl.BlockSpec(memory_space=pltpu.VMEM),
        scratch_shapes=[
            pltpu.VMEM((B_LOC, SQ, DM), F32),
            pltpu.VMEM((DM, 256), F32),
            pltpu.VMEM((256, DM), F32),
            pltpu.VMEM((4, 2, B_LOC, 128, SQ), F32),
            pltpu.VMEM((4, 2, B_LOC, 128, SQ), F32),
            pltpu.VMEM((B_LOC, SQ // 2, DM), I32),
            pltpu.VMEM((2, 2, 8 * NV, 128), I32),
            pltpu.VMEM((2, 4, 2, 4 * NV, 128), I32),
            pltpu.VMEM((2, 4, 2, EXP_ROWS, 128), I32),
            pltpu.VMEM((2, 4, 2, 8 * NV, 128), I32),
            pltpu.VMEM((4, 2, B_LOC, SQ // 2, 128), I32),
            pltpu.VMEM((B_LOC, SQ, DM), F32),
            pltpu.VMEM((4, 2, 2, 8 * NV, 128), I32),
            pltpu.SemaphoreType.DMA((N_LOADS,)),
            pltpu.SemaphoreType.DMA((2, N_COPIES)),
            pltpu.SemaphoreType.DMA((2, N_COPIES)),
            pltpu.SemaphoreType.DMA((2, 2)),
            pltpu.SemaphoreType.DMA((2, 2)),
            pltpu.SemaphoreType.REGULAR,
            pltpu.SemaphoreType.REGULAR,
        ],
        compiler_params=pltpu.CompilerParams(
            collective_id=0,
            disable_semaphore_checks=True,
            vmem_limit_bytes=48 * 1024 * 1024,
            flags={"XLA_TPU_RESCHEDULE_DMA_DONES": True},
        ),
    )(x, Wq, kt, vt, Wo)
```
